```python
import numpy as np

kernel_name = "dist_pipemlp_pp2tp2_xy_b4096_d256_h512"

def setup_inputs():
    x_padded = np.zeros((2, 4096, 256), dtype=np.float32)
    x_padded[0] = np.random.randn(4096, 256).astype(np.float32)
    Win = np.random.randn(4, 256, 1024).astype(np.float32)
    Wout = np.random.randn(4, 1024, 256).astype(np.float32)
    return {"x_padded": x_padded, "Win": Win, "Wout": Wout}

def reference(x_padded, Win, Wout):
    a = x_padded[0]
    for k in range(4):
        h = a @ Win[k]
        h = np.maximum(h, 0.0)
        a = h @ Wout[k]
    out = np.zeros_like(x_padded)
    out[1] = a
    return out
```

```python
import contextlib

import jax
import jax.numpy as jnp
from jax import lax
from jax.experimental import pallas as pl
from jax.experimental.pallas import tpu as pltpu

D = 256
HH = 512
ROWS = 4096
R = ROWS // 2

CFG = dict(
    first=48,
    xb=512,
    m=64,
    late=8,
    late_every=2,
    up0=16,
    w3_pieces=(256, 256),
    share=256,
    early=((128, 512), (128, 512), (128, 768), (128, 768), (128, 768), (128, 256)),
    finish=((256, 128), (384, 256), (640, 128)),
    deferred=((0, 128),),
    fill={1536: (128, 128)},
    steady=(128, 128, 128, 128, 128, 64),
    tail=4,
    detour=((896, 64), (960, 64), (1152, 64), (1216, 64), (1408, 64), (1536, 64), (1664, 32)),
    det_at=30,
    det_early=2,
    det_order="aaaddadaddd" "d",
    scopes=False,
)


def _make_body(cfg):
    first, xb, m = cfg["first"], cfg["xb"], cfg["m"]
    n_xb, n_chunks = R // xb, R // m
    share, det = cfg["share"], cfg["detour"]
    det_parts = len(det)
    up0 = cfg["up0"]
    bf16, f32 = jnp.bfloat16, jnp.float32

    def scope(name):
        return jax.named_scope(name) if cfg["scopes"] else contextlib.nullcontext()

    def loop(lo, hi, step):
        if hi - lo == 1:
            step(lo)
        elif hi > lo:
            lax.fori_loop(lo, hi, lambda i, c: step(i), None)

    def rows(i, n, base=0):
        if isinstance(i, int):
            return pl.ds(base + i * n, n)
        return pl.ds(pl.multiple_of(base + i * n, 16), n)

    def slot(i):
        u = (i - up0) & 3
        moved = i - u + (u >> 1) + 2 * (u & 1)
        if isinstance(i, int):
            return moved if i >= up0 else i
        return jnp.where(i >= up0, moved, i)

    def body(x_hbm, win_hbm, wout_hbm, out_ref,
             wi_f, wo_f, wi, wo, xf, acc, sbuf, ybuf, abuf, h1, h2,
             ld_sem, w_ssem, w_rsem, y_ssem, y_rsem, a_ssem, a_rsem,
             h_ssem, h1_rsem, h2_rsem, h3_rsem, up_ssem, up_rsem, ready):
        mx = lax.axis_index("x")
        my = lax.axis_index("y")
        y_nbr = (mx, 1 - my)
        x_nbr = (1 - mx, my)
        own0 = my * R
        oth0 = (1 - my) * R

        def remote(src, dst, ssem, rsem, dev):
            return pltpu.make_async_remote_copy(
                src, dst, ssem, rsem, device_id=dev,
                device_id_type=pl.DeviceIdType.MESH)

        def mlp(v, s, lo, hi):
            h = jnp.dot(v, wi[s, :, lo:hi], preferred_element_type=f32)
            h = jnp.maximum(h, 0.0).astype(bf16)
            return jnp.dot(h, wo[s, lo:hi, :], preferred_element_type=f32)

        def signal(sem, dev):
            pl.semaphore_signal(sem, inc=1, device_id=dev,
                                device_id_type=pl.DeviceIdType.MESH)

        barrier = pltpu.get_barrier_semaphore()
        signal(barrier, y_nbr)
        pl.when(mx == 0)(lambda: signal(barrier, x_nbr))

        layer = (1 - mx, mx)

        def load_wi(s, r0, n, k):
            return pltpu.make_async_copy(win_hbm.at[layer[s], pl.ds(r0, n)],
                                         wi_f.at[s, pl.ds(r0, n)], ld_sem.at[k])

        def load_wo(s, k):
            return pltpu.make_async_copy(wout_hbm.at[layer[s]], wo_f.at[s], ld_sem.at[k])

        def load_x(b):
            src0 = jnp.where(b < n_xb, oth0 + b * xb, own0 + (b - n_xb) * xb)
            return pltpu.make_async_copy(
                x_hbm.at[0, pl.ds(pl.multiple_of(src0, xb), xb)],
                xf.at[rows(b, xb)], ld_sem.at[5 + b])

        def cast_wi(s, r0, n):
            wi[s, r0:r0 + n, 0:HH] = wi_f[s, r0:r0 + n, :].astype(bf16)

        def cast_wo(s):
            wo[s, 0:HH, :] = wo_f[s].astype(bf16)

        def swap_wi(s, r0, n, c0, nc, k):
            return remote(wi.at[s, pl.ds(r0, n), pl.ds(c0, nc)],
                          wi.at[s, pl.ds(r0, n), pl.ds(HH + c0, nc)],
                          w_ssem.at[k], w_rsem.at[k], y_nbr)

        def swap_wo(s, r0, n, k):
            return remote(wo.at[s, pl.ds(r0, n)], wo.at[s, pl.ds(HH + r0, n)],
                          w_ssem.at[k], w_rsem.at[k], y_nbr)

        loads = [load_wi(0, 0, first, 0), load_wi(0, first, D - first, 1),
                 load_wi(1, 0, D, 2), load_wo(1, 3), load_wo(0, 4)]
        swaps = [swap_wi(0, 0, first, 0, HH, 0), swap_wi(0, first, D - first, 0, HH, 1),
                 swap_wo(0, 0, HH, 2)]
        for c in loads[:4]:
            c.start()
        loads[0].wait()
        cast_wi(0, 0, first)
        with scope("barrier"):
            pl.semaphore_wait(barrier, 1 + mx)
        swaps[0].start()
        pl.when(mx == 1)(lambda: signal(ready, x_nbr))

        @pl.when(mx == 0)
        def _():
            load_x(0).start()

        loads[4].start()

        @pl.when(mx == 0)
        def _():
            for b in range(1, 2 * n_xb):
                load_x(b).start()

        with scope("ld1"):
            loads[1].wait()
        cast_wi(0, first, D - first)
        swaps[1].start()

        def lift(half):
            cols = pl.ds(half * HH, HH)
            return [remote(wi.at[0, :, cols], wi.at[2, :, cols],
                           up_ssem.at[2 * half], up_rsem.at[2 * half], x_nbr),
                    remote(wo.at[0, cols], wo.at[2, cols],
                           up_ssem.at[2 * half + 1], up_rsem.at[2 * half + 1], x_nbr)]

        lifts = lift(0) + lift(1)
        pl.when(mx == 1)(lifts[0].start)
        loads[2].wait()
        cast_wi(1, 0, D)
        loads[3].wait()
        cast_wo(1)

        def finish_first_swap():
            loads[4].wait()
            cast_wo(0)
            swaps[2].start()

        def y_copy(i):
            return remote(sbuf.at[rows(i, m)], ybuf.at[rows(i, m)],
                          y_ssem.at[i], y_rsem.at[i], y_nbr)

        def act_copy(i):
            return remote(abuf.at[rows(i, m)], abuf.at[rows(i, m)],
                          a_ssem.at[i], a_rsem.at[i], x_nbr)

        def detour(j, hop):
            part, res = pl.ds(sum(n for _, n in det[:j]), det[j][1]), pl.ds(*det[j])
            if hop == 0:
                return remote(sbuf.at[res], h1.at[part],
                              h_ssem.at[j], h1_rsem.at[j], x_nbr)
            if hop == 1:
                return remote(h1.at[part], h2.at[part],
                              h_ssem.at[j], h2_rsem.at[j], y_nbr)
            return remote(h2.at[part], ybuf.at[res],
                          h_ssem.at[det_parts + j], h3_rsem.at[j], x_nbr)

        @pl.when(mx == 0)
        def _stage0():
            late = cfg["late"]

            def layer0(r):
                return mlp(xf[r, :].astype(bf16), 1, 0, HH)

            def l0_step(b):
                with scope("xw"):
                    load_x(b).wait()
                part = layer0(rows(b, xb))
                acc[rows(b, xb), :] = part
                sbuf[rows(b, xb), :] = part.astype(bf16)

                pl.when(b == 0)(finish_first_swap)

                @pl.when(b < n_xb)
                def _():
                    for i in range(xb // m):
                        y_copy(slot(b * (xb // m) + i)).start()

            n_full = (ROWS - late * m) // xb
            loop(0, n_full, l0_step)
            for b in range(n_full, 2 * n_xb):
                load_x(b).wait()
            rest = ROWS - late * m - n_full * xb
            if rest:
                acc[pl.ds(n_full * xb, rest), :] = layer0(pl.ds(n_full * xb, rest))

            pl.semaphore_wait(ready, 1)
            with scope("w1_wait"):
                for c in swaps:
                    c.wait_recv()

            def l1_step(i, with_l0=False, with_l2=False):
                k = slot(i)
                with scope("pw"):
                    y_copy(k).wait_recv()
                a = acc[rows(k, m, R), :] + ybuf[rows(k, m), :].astype(f32)
                a = mlp(a.astype(bf16), 0, 0, 2 * HH).astype(bf16)
                if with_l2:
                    if isinstance(i, int) and i == up0 + 1:
                        with scope("up_wait"):
                            for c in lifts:
                                c.wait_recv()
                    a = mlp(a, 2, 0, 2 * HH).astype(bf16)
                abuf[rows(k, m), :] = a
                act_copy(k).start()
                out_ref[0, rows(i, 2 * m), :] = jnp.zeros((2 * m, D), f32)
                if with_l0:
                    @pl.when(lax.rem(i, every) == 0)
                    def _():
                        r = rows(lax.div(i, every), m, ROWS - late * m)
                        acc[r, :] = layer0(r)

            def l1_pair(p):
                l1_step(2 * p)
                l1_step(2 * p + 1, with_l2=True)

            def l1_range(lo, hi):
                loop(lo, min(hi, up0), l1_step)
                loop(max(lo, up0) // 2, hi // 2, l1_pair)

            def pass_on(lo, hi):
                for j in range(lo, hi):
                    with scope("det1"):
                        detour(j, 0).wait_recv()
                    detour(j, 1).start()

            every = cfg["late_every"]
            loop(0, late * every, lambda i: l1_step(i, with_l0=True))
            l1_range(late * every, up0)
            l1_range(up0, up0 + 2)
            l1_range(up0 + 2, cfg["det_at"])
            pass_on(0, cfg["det_early"])
            l1_range(cfg["det_at"], n_chunks)
            across, down = cfg["det_early"], 0
            for op in cfg["det_order"]:
                if op == "a":
                    pass_on(across, across + 1)
                    across += 1
                else:
                    with scope("det2"):
                        detour(down, 1).wait_recv()
                    detour(down, 2).start()
                    down += 1
            assert across == down == det_parts
            with scope("drain"):
                for c in swaps:
                    c.wait_send()

                def drain(i):
                    y_copy(i).wait_send()
                    act_copy(i).wait_send()

                loop(0, n_chunks, drain)
                for j in range(det_parts):
                    detour(j, 1).wait_send()
                    detour(j, 2).wait_send()

        @pl.when(mx == 1)
        def _stage1():
            finish_first_swap()
            lifts[1].start()
            w3_swaps = []
            c0 = 0
            for k, nc in enumerate(cfg["w3_pieces"]):
                pair = [swap_wi(1, 0, D, c0, nc, 3 + 2 * k), swap_wo(1, c0, nc, 4 + 2 * k)]
                for c in pair:
                    c.start()
                c0 += nc
                w3_swaps.append((HH + c0, pair))
            all_swaps = swaps + [c for _, pair in w3_swaps for c in pair]
            have = [HH]

            def need_w3(hidden):
                while have[0] < hidden:
                    have[0], pair = w3_swaps.pop(0)
                    for k, c in enumerate(pair):
                        with scope("w3_wait%d" % k):
                            c.wait_recv()

            def write_out(col0, r0, n, val):
                out_ref[0, pl.ds(pl.multiple_of(col0 + r0, 8), n), :] = val.astype(f32)

            sent = []

            def send(r0, n):
                k = len(sent)
                sent.append((r0, n, remote(sbuf.at[pl.ds(r0, n)], ybuf.at[pl.ds(r0, n)],
                                           y_ssem.at[k], y_rsem.at[k], y_nbr)))
                sent[k][2].start()

            def emit(r0, n, res):
                res = res.astype(bf16)
                if r0 >= share:
                    sbuf[r0:r0 + n, :] = res
                    r = r0
                    for j, (d0, dn) in enumerate(det):
                        if r0 <= d0 < r0 + n:
                            if r < d0:
                                send(r, d0 - r)
                            detour(j, 0).start()
                            r = d0 + dn
                    if r < r0 + n:
                        send(r, r0 + n - r)
                write_out(own0, r0, n, res)

            def take(copies):
                with scope("rw"):
                    for _, _, c in copies:
                        c.wait_recv()
                for r0, n, _ in copies:
                    write_out(oth0, r0, n, ybuf[r0:r0 + n, :])

            def arrived(r0, n):
                with scope("aw"):
                    for i in range(r0 // m, (r0 + n) // m):
                        act_copy(i).wait_recv()

            def layer2(r0, n):
                return mlp(abuf[r0:r0 + n, :], 0, 0, 2 * HH).astype(bf16)

            with scope("w2_wait"):
                for c in swaps:
                    c.wait_recv()
            for c in lifts[2:]:
                c.start()

            done = {}
            r0 = 0
            for n, hid in cfg["early"]:
                need_w3(hid)
                arrived(r0, n)
                a3 = layer2(r0, n)
                abuf[r0:r0 + n, :] = a3
                if r0 < share:
                    sbuf[r0:r0 + n, :] = a3
                    send(r0, n)
                if hid:
                    acc[r0:r0 + n, :] = mlp(a3, 1, 0, hid)
                done.update({k: hid for k in range(r0 // m, (r0 + n) // m)})
                r0 += n
            taken = len(sent)
            need_w3(2 * HH)

            def finish(r0, n):
                hid = done[r0 // m]
                assert all(done.pop(k) == hid for k in range(r0 // m, (r0 + n) // m))
                res = mlp(abuf[r0:r0 + n, :], 1, hid, 2 * HH)
                emit(r0, n, acc[r0:r0 + n, :] + res if hid else res)

            for group in cfg["finish"]:
                with scope("fin"):
                    finish(*group)

            for n in cfg["steady"]:
                if r0 < up0 * m:
                    arrived(r0, n)
                    emit(r0, n, mlp(layer2(r0, n), 1, 0, 2 * HH))
                    r0 += n
                    continue
                if r0 in cfg["fill"]:
                    finish(*cfg["fill"][r0])
                for lo in range(r0, r0 + 2 * m, n):
                    arrived(lo, n)
                    emit(lo, n, mlp(layer2(lo, n), 1, 0, 2 * HH))
                    arrived(lo + 2 * m, n)
                    emit(lo + 2 * m, n, mlp(abuf[lo + 2 * m:lo + 2 * m + n, :], 1, 0, 2 * HH))
                r0 += 4 * m
            assert r0 == R
            before = len(sent) - cfg["tail"]
            with scope("shared"):
                for _, _, c in sent[:before]:
                    c.wait_recv()
            for r0, n, _ in sent[taken:before]:
                write_out(oth0, r0, n, ybuf[r0:r0 + n, :])
            for group in cfg["deferred"]:
                finish(*group)
            res = mlp(ybuf[0:share, :], 1, 0, 2 * HH)
            write_out(oth0, 0, share, res.astype(bf16))
            assert not done
            taken = before
            for j in range(det_parts):
                upto = before + (j * cfg["tail"]) // det_parts
                for c in sent[taken:upto]:
                    take([c])
                taken = upto
                if j == det_parts - 1:
                    with scope("drain"):
                        for c in all_swaps + lifts + [c for _, _, c in sent[:-1]]:
                            c.wait_send()
                        for i in range(det_parts):
                            detour(i, 0).wait_send()
                with scope("hw"):
                    detour(j, 2).wait_recv()
                write_out(oth0, *det[j], ybuf[pl.ds(*det[j]), :])
            sent[-1][2].wait_send()
            for c in sent[taken:]:
                take([c])
            with scope("end"):
                pass

    return body


def _build(cfg):
    n_chunks = R // cfg["m"]
    det_parts, det_rows = len(cfg["detour"]), sum(n for _, n in cfg["detour"])
    n_w = 3 + 2 * len(cfg["w3_pieces"])
    dma = pltpu.SemaphoreType.DMA
    bf16, f32 = jnp.bfloat16, jnp.float32
    return pl.pallas_call(
        _make_body(cfg),
        out_shape=pltpu.VMEM((1, ROWS, D), f32),
        in_specs=[pl.BlockSpec(memory_space=pltpu.HBM)] * 3,
        out_specs=pl.BlockSpec(memory_space=pltpu.VMEM),
        scratch_shapes=[
            pltpu.VMEM((2, D, HH), f32),
            pltpu.VMEM((2, HH, D), f32),
            pltpu.VMEM((3, D, 2 * HH), bf16),
            pltpu.VMEM((3, 2 * HH, D), bf16),
            pltpu.VMEM((ROWS, D), f32),
            pltpu.VMEM((ROWS, D), f32),
            pltpu.VMEM((ROWS, D), bf16),
            pltpu.VMEM((R, D), bf16),
            pltpu.VMEM((R, D), bf16),
            pltpu.VMEM((det_rows, D), bf16),
            pltpu.VMEM((det_rows, D), bf16),
            dma((5 + ROWS // cfg["xb"],)),
            dma((n_w,)), dma((n_w,)),
            dma((n_chunks,)), dma((n_chunks,)),
            dma((n_chunks,)), dma((n_chunks,)),
            dma((2 * det_parts,)), dma((det_parts,)), dma((det_parts,)), dma((det_parts,)),
            dma((4,)), dma((4,)), pltpu.SemaphoreType.REGULAR,
        ],
        compiler_params=pltpu.CompilerParams(
            collective_id=0, vmem_limit_bytes=32 * 1024 * 1024,
            disable_semaphore_checks=True),
    )


def pallas_dist_pipemlp_pp2tp2_xy_b4096_d256_h512_kernel(
    x_padded: jax.Array,
    Win: jax.Array,
    Wout: jax.Array,
):
    return _build(CFG)(x_padded, Win, Wout)
```

```python
import jax
import jax.numpy as jnp
from jax import lax
from jax.experimental import pallas as pl
from jax.experimental.pallas import tpu as pltpu

D = 256
HH = 512
ROWS = 4096
R = ROWS // 2

FIRST = 48
XB = 512
M = 64
N_CHUNKS = R // M
UP0 = 16

SHARE = 256
EARLY = ((128, HH),) * 5 + ((128, HH // 2),)
FINISH = ((256, 128), (384, 256), (640, 128))
STEADY = (128, 128, 128, 128, 64, 64)
DETOUR = ((896, 64), (960, 64), (1152, 64), (1216, 64), (1408, 64), (1536, 64), (1664, 32))
DET_AT = 30
DET_EARLY = 2
DET_ORDER = "aaaddadadddd"
TAIL = 6

BF16, F32 = jnp.bfloat16, jnp.float32


def _loop(lo, hi, step):
    if hi - lo == 1:
        step(lo)
    else:
        lax.fori_loop(lo, hi, lambda i, carry: step(i), None)


def _rows(i, n, base=0):
    if isinstance(i, int):
        return pl.ds(base + i * n, n)
    return pl.ds(pl.multiple_of(base + i * n, M), n)


def _slot(i):
    u = (i - UP0) & 3
    moved = i - u + (u >> 1) + 2 * (u & 1)
    if isinstance(i, int):
        return moved if i >= UP0 else i
    return jnp.where(i >= UP0, moved, i)


def _body(x_hbm, win_hbm, wout_hbm, out_ref,
          wi_f, wo_f, wi, wo, xf, acc, sbuf, ybuf, abuf, h1, h2,
          ld_sem, w_ssem, w_rsem, up_ssem, up_rsem, y_ssem, y_rsem, a_ssem, a_rsem,
          h_ssem, h1_rsem, h2_rsem, h3_rsem, ready):
    mx = lax.axis_index("x")
    my = lax.axis_index("y")
    y_nbr = (mx, 1 - my)
    x_nbr = (1 - mx, my)
    own0 = my * R
    oth0 = (1 - my) * R
    n_xb = R // XB
    n_det = len(DETOUR)

    def remote(src, dst, ssem, rsem, dev):
        return pltpu.make_async_remote_copy(
            src, dst, ssem, rsem, device_id=dev, device_id_type=pl.DeviceIdType.MESH)

    def signal(sem, dev):
        pl.semaphore_signal(sem, inc=1, device_id=dev, device_id_type=pl.DeviceIdType.MESH)

    def mlp(v, s, lo=0, hi=2 * HH):
        h = jnp.dot(v, wi[s, :, lo:hi], preferred_element_type=F32)
        h = jnp.maximum(h, 0.0).astype(BF16)
        return jnp.dot(h, wo[s, lo:hi, :], preferred_element_type=F32)

    barrier = pltpu.get_barrier_semaphore()
    signal(barrier, y_nbr)
    pl.when(mx == 0)(lambda: signal(barrier, x_nbr))

    layer = (1 - mx, mx)

    def load_wi(s, r0, n, k):
        return pltpu.make_async_copy(win_hbm.at[layer[s], pl.ds(r0, n)],
                                     wi_f.at[s, pl.ds(r0, n)], ld_sem.at[k])

    def load_wo(s, k):
        return pltpu.make_async_copy(wout_hbm.at[layer[s]], wo_f.at[s], ld_sem.at[k])

    def load_x(b):
        src0 = jnp.where(b < n_xb, oth0 + b * XB, own0 + (b - n_xb) * XB)
        return pltpu.make_async_copy(x_hbm.at[0, pl.ds(pl.multiple_of(src0, XB), XB)],
                                     xf.at[_rows(b, XB)], ld_sem.at[5 + b])

    def cast_wi(s, r0, n):
        wi[s, r0:r0 + n, 0:HH] = wi_f[s, r0:r0 + n, :].astype(BF16)

    def cast_wo(s):
        wo[s, 0:HH, :] = wo_f[s].astype(BF16)

    def swap_wi(s, r0, n, k):
        return remote(wi.at[s, pl.ds(r0, n), pl.ds(0, HH)], wi.at[s, pl.ds(r0, n), pl.ds(HH, HH)],
                      w_ssem.at[k], w_rsem.at[k], y_nbr)

    def swap_wo(s, k):
        return remote(wo.at[s, pl.ds(0, HH)], wo.at[s, pl.ds(HH, HH)],
                      w_ssem.at[k], w_rsem.at[k], y_nbr)

    def lift(half):
        units = pl.ds(half * HH, HH)
        return [remote(wi.at[0, pl.ds(0, D), units], wi.at[2, pl.ds(0, D), units],
                       up_ssem.at[2 * half], up_rsem.at[2 * half], x_nbr),
                remote(wo.at[0, units], wo.at[2, units],
                       up_ssem.at[2 * half + 1], up_rsem.at[2 * half + 1], x_nbr)]

    loads = [load_wi(0, 0, FIRST, 0), load_wi(0, FIRST, D - FIRST, 1),
             load_wi(1, 0, D, 2), load_wo(1, 3), load_wo(0, 4)]
    swaps = [swap_wi(0, 0, FIRST, 0), swap_wi(0, FIRST, D - FIRST, 1), swap_wo(0, 2)]
    lifts = lift(0) + lift(1)

    for c in loads[:4]:
        c.start()
    loads[0].wait()
    cast_wi(0, 0, FIRST)
    pl.when(mx == 0)(lambda: pl.semaphore_wait(barrier, 1))
    pl.when(mx == 1)(lambda: pl.semaphore_wait(barrier, 2))
    swaps[0].start()
    pl.when(mx == 1)(lambda: signal(ready, x_nbr))
    pl.when(mx == 0)(lambda: load_x(0).start())
    loads[4].start()

    @pl.when(mx == 0)
    def _():
        for b in range(1, 2 * n_xb):
            load_x(b).start()

    loads[1].wait()
    cast_wi(0, FIRST, D - FIRST)
    swaps[1].start()
    pl.when(mx == 1)(lambda: lifts[0].start())
    loads[2].wait()
    cast_wi(1, 0, D)
    loads[3].wait()
    cast_wo(1)

    def finish_first_swap():
        loads[4].wait()
        cast_wo(0)
        swaps[2].start()

    def part_copy(k):
        return remote(sbuf.at[_rows(k, M)], ybuf.at[_rows(k, M)],
                      y_ssem.at[k], y_rsem.at[k], y_nbr)

    def act_copy(k):
        return remote(abuf.at[_rows(k, M)], abuf.at[_rows(k, M)],
                      a_ssem.at[k], a_rsem.at[k], x_nbr)

    def detour(j, hop):
        part = pl.ds(sum(n for _, n in DETOUR[:j]), DETOUR[j][1])
        res = pl.ds(*DETOUR[j])
        if hop == 0:
            return remote(sbuf.at[res], h1.at[part], h_ssem.at[j], h1_rsem.at[j], x_nbr)
        if hop == 1:
            return remote(h1.at[part], h2.at[part], h_ssem.at[j], h2_rsem.at[j], y_nbr)
        return remote(h2.at[part], ybuf.at[res],
                      h_ssem.at[n_det + j], h3_rsem.at[j], x_nbr)

    @pl.when(mx == 0)
    def _stage0():
        def layer0(r):
            return mlp(xf[r, :].astype(BF16), 1, 0, HH)

        def l0_step(b):
            load_x(b).wait()
            part = layer0(_rows(b, XB))
            acc[_rows(b, XB), :] = part
            sbuf[_rows(b, XB), :] = part.astype(BF16)
            pl.when(b == 0)(finish_first_swap)

            @pl.when(b < n_xb)
            def _():
                for i in range(XB // M):
                    part_copy(_slot(b * (XB // M) + i)).start()

        _loop(0, 2 * n_xb - 1, l0_step)
        load_x(2 * n_xb - 1).wait()

        pl.semaphore_wait(ready, 1)
        for c in swaps:
            c.wait_recv()

        def l1_step(i, with_l0=False, with_l2=False):
            k = _slot(i)
            part_copy(k).wait_recv()
            a = acc[_rows(k, M, R), :] + ybuf[_rows(k, M), :].astype(F32)
            a = mlp(a.astype(BF16), 0).astype(BF16)
            if with_l2:
                if isinstance(i, int) and i == UP0 + 1:
                    for c in lifts:
                        c.wait_recv()
                a = mlp(a, 2).astype(BF16)
            abuf[_rows(k, M), :] = a
            act_copy(k).start()
            out_ref[0, _rows(i, 2 * M), :] = jnp.zeros((2 * M, D), F32)
            if with_l0:
                @pl.when((i & 1) == 0)
                def _():
                    r = _rows(i >> 1, M, ROWS - XB)
                    acc[r, :] = layer0(r)

        def l1_pair(p):
            l1_step(2 * p)
            l1_step(2 * p + 1, with_l2=True)

        def pass_across(j):
            detour(j, 0).wait_recv()
            detour(j, 1).start()

        assert UP0 == 2 * XB // M
        _loop(0, UP0, lambda i: l1_step(i, with_l0=True))
        l1_pair(UP0 // 2)
        _loop(UP0 // 2 + 1, DET_AT // 2, l1_pair)
        for j in range(DET_EARLY):
            pass_across(j)
        _loop(DET_AT // 2, N_CHUNKS // 2, l1_pair)
        across, down = DET_EARLY, 0
        for op in DET_ORDER:
            if op == "a":
                pass_across(across)
                across += 1
            else:
                detour(down, 1).wait_recv()
                detour(down, 2).start()
                down += 1
        assert across == down == n_det

        def drain(k):
            part_copy(k).wait_send()
            act_copy(k).wait_send()

        for c in swaps:
            c.wait_send()
        _loop(0, N_CHUNKS, drain)
        for j in range(n_det):
            detour(j, 1).wait_send()
            detour(j, 2).wait_send()

    @pl.when(mx == 1)
    def _stage1():
        finish_first_swap()
        lifts[1].start()
        w3_swaps = [swap_wi(1, 0, D, 3), swap_wo(1, 4)]
        for c in w3_swaps:
            c.start()

        def write_out(col0, r0, n, val):
            out_ref[0, pl.ds(pl.multiple_of(col0 + r0, 8), n), :] = val.astype(F32)

        sent = []

        def send(r0, n):
            k = len(sent)
            assert k < N_CHUNKS
            c = remote(sbuf.at[pl.ds(r0, n)], ybuf.at[pl.ds(r0, n)],
                       y_ssem.at[k], y_rsem.at[k], y_nbr)
            c.start()
            sent.append((r0, n, c))

        def emit(r0, n, res):
            if r0 >= SHARE:
                sbuf[r0:r0 + n, :] = res.astype(BF16)
                r = r0
                for j, (d0, dn) in enumerate(DETOUR):
                    if r0 <= d0 < r0 + n:
                        if r < d0:
                            send(r, d0 - r)
                        detour(j, 0).start()
                        r = d0 + dn
                assert r <= r0 + n
                if r < r0 + n:
                    send(r, r0 + n - r)
            write_out(own0, r0, n, res)

        def arrived(r0, n):
            for k in range(r0 // M, (r0 + n) // M):
                act_copy(k).wait_recv()

        def layer2(r0, n):
            return mlp(abuf[r0:r0 + n, :], 0).astype(BF16)

        for c in swaps:
            c.wait_recv()
        for c in lifts[2:]:
            c.start()

        applied = {}
        r0 = 0
        for n, hid in EARLY:
            arrived(r0, n)
            a3 = layer2(r0, n)
            abuf[r0:r0 + n, :] = a3
            if r0 < SHARE:
                sbuf[r0:r0 + n, :] = a3
                send(r0, n)
            acc[r0:r0 + n, :] = mlp(a3, 1, 0, hid)
            applied.update({k: hid for k in range(r0 // M, (r0 + n) // M)})
            r0 += n
        n_shared = len(sent)
        for c in w3_swaps:
            c.wait_recv()

        def finish(f0, n):
            hid = applied[f0 // M]
            assert all(applied.pop(k) == hid for k in range(f0 // M, (f0 + n) // M))
            emit(f0, n, acc[f0:f0 + n, :] + mlp(abuf[f0:f0 + n, :], 1, hid))

        for f0, n in FINISH:
            finish(f0, n)

        for n in STEADY:
            if r0 < UP0 * M:
                arrived(r0, n)
                emit(r0, n, mlp(layer2(r0, n), 1))
                r0 += n
                continue
            for lo in range(r0, r0 + 2 * M, n):
                arrived(lo, n)
                emit(lo, n, mlp(layer2(lo, n), 1))
                arrived(lo + 2 * M, n)
                emit(lo + 2 * M, n, mlp(abuf[lo + 2 * M:lo + 2 * M + n, :], 1))
            r0 += 4 * M
        assert r0 == R

        before = len(sent) - TAIL
        for _, _, c in sent[:before]:
            c.wait_recv()
        for p0, n, _ in sent[n_shared:before]:
            write_out(oth0, p0, n, ybuf[p0:p0 + n, :])
        finish(0, SHARE)
        write_out(oth0, 0, SHARE, mlp(ybuf[0:SHARE, :], 1))
        assert not applied

        def take(p0, n, c):
            c.wait_recv()
            write_out(oth0, p0, n, ybuf[p0:p0 + n, :])

        taken = before
        for j in range(n_det):
            upto = before + (j * TAIL) // n_det
            for piece in sent[taken:upto]:
                take(*piece)
            taken = upto
            if j == n_det - 1:
                for c in swaps + w3_swaps + lifts + [c for _, _, c in sent[:-1]]:
                    c.wait_send()
                for i in range(n_det):
                    detour(i, 0).wait_send()
            take(*DETOUR[j], detour(j, 2))
        sent[-1][2].wait_send()
        for piece in sent[taken:]:
            take(*piece)


def pallas_dist_pipemlp_pp2tp2_xy_b4096_d256_h512_kernel(
    x_padded: jax.Array,
    Win: jax.Array,
    Wout: jax.Array,
):
    n_det = len(DETOUR)
    det_rows = sum(n for _, n in DETOUR)
    dma = pltpu.SemaphoreType.DMA
    return pl.pallas_call(
        _body,
        out_shape=pltpu.VMEM((1, ROWS, D), F32),
        in_specs=[pl.BlockSpec(memory_space=pltpu.HBM)] * 3,
        out_specs=pl.BlockSpec(memory_space=pltpu.VMEM),
        scratch_shapes=[
            pltpu.VMEM((2, D, HH), F32),
            pltpu.VMEM((2, HH, D), F32),
            pltpu.VMEM((3, D, 2 * HH), BF16),
            pltpu.VMEM((3, 2 * HH, D), BF16),
            pltpu.VMEM((ROWS, D), F32),
            pltpu.VMEM((ROWS, D), F32),
            pltpu.VMEM((ROWS, D), BF16),
            pltpu.VMEM((R, D), BF16),
            pltpu.VMEM((R, D), BF16),
            pltpu.VMEM((det_rows, D), BF16),
            pltpu.VMEM((det_rows, D), BF16),
            dma((5 + ROWS // XB,)),
            dma((5,)), dma((5,)),
            dma((4,)), dma((4,)),
            dma((N_CHUNKS,)), dma((N_CHUNKS,)),
            dma((N_CHUNKS,)), dma((N_CHUNKS,)),
            dma((2 * n_det,)), dma((n_det,)), dma((n_det,)), dma((n_det,)),
            pltpu.SemaphoreType.REGULAR,
        ],
        compiler_params=pltpu.CompilerParams(
            collective_id=0,
            vmem_limit_bytes=32 * 1024 * 1024,
            disable_semaphore_checks=True,
        ),
    )(x_padded, Win, Wout)
```

```python
import jax
import jax.numpy as jnp
from jax import lax
from jax.experimental import pallas as pl
from jax.experimental.pallas import tpu as pltpu

D = 256
HH = 512
ROWS = 4096
R = ROWS // 2

FIRST = (16, 48, 192)
XB = 512
M = 64
N_CHUNKS = R // M
UP0 = 16

SHARE = 256
EARLY = ((128, HH),) * 5 + ((128, HH // 2),)
FINISH = ((256, 128), (384, 256), (640, 128))
STEADY = (128, 128, 128, 128, 64, 64)
DETOUR = ((896, 64), (960, 64), (1152, 64), (1216, 64), (1408, 64), (1536, 64), (1664, 32))
DET_AT = 30
DET_EARLY = 2
DET_ORDER = "aaaddadadddd"
TAIL = 6

BF16, F32 = jnp.bfloat16, jnp.float32


def _loop(lo, hi, step):
    if hi - lo == 1:
        step(lo)
    else:
        lax.fori_loop(lo, hi, lambda i, carry: step(i), None)


def _rows(i, n, base=0):
    if isinstance(i, int):
        return pl.ds(base + i * n, n)
    return pl.ds(pl.multiple_of(base + i * n, M), n)


def _slot(i):
    u = (i - UP0) & 3
    moved = i - u + (u >> 1) + 2 * (u & 1)
    if isinstance(i, int):
        return moved if i >= UP0 else i
    return jnp.where(i >= UP0, moved, i)


def _body(x_hbm, win_hbm, wout_hbm, out_ref,
          wi_f, wo_f, wi, wo, xf, acc, sbuf, ybuf, abuf, h1, h2,
          ld_sem, w_ssem, w_rsem, up_ssem, up_rsem, y_ssem, y_rsem, a_ssem, a_rsem,
          h_ssem, h1_rsem, h2_rsem, h3_rsem, ready):
    mx = lax.axis_index("x")
    my = lax.axis_index("y")
    y_nbr = (mx, 1 - my)
    x_nbr = (1 - mx, my)
    own0 = my * R
    oth0 = (1 - my) * R
    n_xb = R // XB
    n_det = len(DETOUR)

    def remote(src, dst, ssem, rsem, dev):
        return pltpu.make_async_remote_copy(
            src, dst, ssem, rsem, device_id=dev, device_id_type=pl.DeviceIdType.MESH)

    def signal(sem, dev):
        pl.semaphore_signal(sem, inc=1, device_id=dev, device_id_type=pl.DeviceIdType.MESH)

    def mlp(v, s, lo=0, hi=2 * HH):
        h = jnp.dot(v, wi[s, :, lo:hi], preferred_element_type=F32)
        h = jnp.maximum(h, 0.0).astype(BF16)
        return jnp.dot(h, wo[s, lo:hi, :], preferred_element_type=F32)

    layer = (1 - mx, mx)

    def load_wi(s, r0, n, k):
        return pltpu.make_async_copy(win_hbm.at[layer[s], pl.ds(r0, n)],
                                     wi_f.at[s, pl.ds(r0, n)], ld_sem.at[k])

    def load_wo(s, k):
        return pltpu.make_async_copy(wout_hbm.at[layer[s]], wo_f.at[s], ld_sem.at[k])

    def load_x(b):
        src0 = jnp.where(b < n_xb, oth0 + b * XB, own0 + (b - n_xb) * XB)
        return pltpu.make_async_copy(x_hbm.at[0, pl.ds(pl.multiple_of(src0, XB), XB)],
                                     xf.at[_rows(b, XB)], ld_sem.at[len(FIRST) + 3 + b])

    def cast_wi(s, r0, n):
        wi[s, r0:r0 + n, 0:HH] = wi_f[s, r0:r0 + n, :].astype(BF16)

    def cast_wo(s):
        wo[s, 0:HH, :] = wo_f[s].astype(BF16)

    def swap_wi(s, r0, n, k):
        return remote(wi.at[s, pl.ds(r0, n), pl.ds(0, HH)], wi.at[s, pl.ds(r0, n), pl.ds(HH, HH)],
                      w_ssem.at[k], w_rsem.at[k], y_nbr)

    def swap_wo(s, k):
        return remote(wo.at[s, pl.ds(0, HH)], wo.at[s, pl.ds(HH, HH)],
                      w_ssem.at[k], w_rsem.at[k], y_nbr)

    def lift(half):
        units = pl.ds(half * HH, HH)
        return [remote(wi.at[0, pl.ds(0, D), units], wi.at[2, pl.ds(0, D), units],
                       up_ssem.at[2 * half], up_rsem.at[2 * half], x_nbr),
                remote(wo.at[0, units], wo.at[2, units],
                       up_ssem.at[2 * half + 1], up_rsem.at[2 * half + 1], x_nbr)]

    pieces = [(sum(FIRST[:k]), n) for k, n in enumerate(FIRST)]
    n_p = len(pieces)
    first_loads = [load_wi(0, r0, n, k) for k, (r0, n) in enumerate(pieces)]
    loads = [load_wi(1, 0, D, n_p), load_wo(1, n_p + 1), load_wo(0, n_p + 2)]
    swaps = [swap_wi(0, r0, n, k) for k, (r0, n) in enumerate(pieces)] + [swap_wo(0, n_p)]
    lifts = lift(0) + lift(1)

    first_loads[0].start()

    barrier = pltpu.get_barrier_semaphore()
    signal(barrier, y_nbr)
    pl.when(mx == 0)(lambda: signal(barrier, x_nbr))

    for c in first_loads[1:] + loads[:2]:
        c.start()
    pl.when(mx == 0)(lambda: load_x(0).start())
    loads[2].start()

    @pl.when(mx == 0)
    def _():
        for b in range(1, 2 * n_xb):
            load_x(b).start()

    first_loads[0].wait()
    cast_wi(0, *pieces[0])
    pl.when(mx == 0)(lambda: pl.semaphore_wait(barrier, 1))
    pl.when(mx == 1)(lambda: pl.semaphore_wait(barrier, 2))
    swaps[0].start()
    for k in range(1, n_p):
        first_loads[k].wait()
        cast_wi(0, *pieces[k])
        swaps[k].start()
    pl.when(mx == 1)(lambda: signal(ready, x_nbr))
    pl.when(mx == 1)(lambda: lifts[0].start())
    loads[0].wait()
    cast_wi(1, 0, D)
    loads[1].wait()
    cast_wo(1)

    def finish_first_swap():
        loads[2].wait()
        cast_wo(0)
        swaps[n_p].start()

    def part_copy(k):
        return remote(sbuf.at[_rows(k, M)], ybuf.at[_rows(k, M)],
                      y_ssem.at[k], y_rsem.at[k], y_nbr)

    def act_copy(k):
        return remote(abuf.at[_rows(k, M)], abuf.at[_rows(k, M)],
                      a_ssem.at[k], a_rsem.at[k], x_nbr)

    def detour(j, hop):
        part = pl.ds(sum(n for _, n in DETOUR[:j]), DETOUR[j][1])
        res = pl.ds(*DETOUR[j])
        if hop == 0:
            return remote(sbuf.at[res], h1.at[part], h_ssem.at[j], h1_rsem.at[j], x_nbr)
        if hop == 1:
            return remote(h1.at[part], h2.at[part], h_ssem.at[j], h2_rsem.at[j], y_nbr)
        return remote(h2.at[part], ybuf.at[res],
                      h_ssem.at[n_det + j], h3_rsem.at[j], x_nbr)

    @pl.when(mx == 0)
    def _stage0():
        def layer0(r):
            return mlp(xf[r, :].astype(BF16), 1, 0, HH)

        def l0_step(b):
            load_x(b).wait()
            part = layer0(_rows(b, XB))
            acc[_rows(b, XB), :] = part
            sbuf[_rows(b, XB), :] = part.astype(BF16)
            pl.when(b == 0)(finish_first_swap)

            @pl.when(b < n_xb)
            def _():
                for i in range(XB // M):
                    part_copy(_slot(b * (XB // M) + i)).start()

        _loop(0, 2 * n_xb - 1, l0_step)
        load_x(2 * n_xb - 1).wait()

        pl.semaphore_wait(ready, 1)
        for c in swaps:
            c.wait_recv()

        def l1_step(i, with_l0=False, with_l2=False):
            k = _slot(i)
            part_copy(k).wait_recv()
            a = acc[_rows(k, M, R), :] + ybuf[_rows(k, M), :].astype(F32)
            a = mlp(a.astype(BF16), 0).astype(BF16)
            if with_l2:
                if isinstance(i, int) and i == UP0 + 1:
                    for c in lifts:
                        c.wait_recv()
                a = mlp(a, 2).astype(BF16)
            abuf[_rows(k, M), :] = a
            act_copy(k).start()
            out_ref[0, _rows(i, 2 * M), :] = jnp.zeros((2 * M, D), F32)
            if with_l0:
                @pl.when((i & 1) == 0)
                def _():
                    r = _rows(i >> 1, M, ROWS - XB)
                    acc[r, :] = layer0(r)

        def l1_pair(p):
            l1_step(2 * p)
            l1_step(2 * p + 1, with_l2=True)

        def pass_across(j):
            detour(j, 0).wait_recv()
            detour(j, 1).start()

        assert UP0 == 2 * XB // M
        _loop(0, UP0, lambda i: l1_step(i, with_l0=True))
        l1_pair(UP0 // 2)
        _loop(UP0 // 2 + 1, DET_AT // 2, l1_pair)
        for j in range(DET_EARLY):
            pass_across(j)
        _loop(DET_AT // 2, N_CHUNKS // 2, l1_pair)
        across, down = DET_EARLY, 0
        for op in DET_ORDER:
            if op == "a":
                pass_across(across)
                across += 1
            else:
                detour(down, 1).wait_recv()
                detour(down, 2).start()
                down += 1
        assert across == down == n_det

        def drain(k):
            part_copy(k).wait_send()
            act_copy(k).wait_send()

        for c in swaps:
            c.wait_send()
        _loop(0, N_CHUNKS, drain)
        for j in range(n_det):
            detour(j, 1).wait_send()
            detour(j, 2).wait_send()

    @pl.when(mx == 1)
    def _stage1():
        finish_first_swap()
        lifts[1].start()
        w3_swaps = [swap_wi(1, 0, D, n_p + 1), swap_wo(1, n_p + 2)]
        for c in w3_swaps:
            c.start()

        def write_out(col0, r0, n, val):
            out_ref[0, pl.ds(pl.multiple_of(col0 + r0, 8), n), :] = val.astype(F32)

        sent = []

        def send(r0, n):
            k = len(sent)
            assert k < N_CHUNKS
            c = remote(sbuf.at[pl.ds(r0, n)], ybuf.at[pl.ds(r0, n)],
                       y_ssem.at[k], y_rsem.at[k], y_nbr)
            c.start()
            sent.append((r0, n, c))

        def emit(r0, n, res):
            if r0 >= SHARE:
                sbuf[r0:r0 + n, :] = res.astype(BF16)
                r = r0
                for j, (d0, dn) in enumerate(DETOUR):
                    if r0 <= d0 < r0 + n:
                        if r < d0:
                            send(r, d0 - r)
                        detour(j, 0).start()
                        r = d0 + dn
                assert r <= r0 + n
                if r < r0 + n:
                    send(r, r0 + n - r)
            write_out(own0, r0, n, res)

        def arrived(r0, n):
            for k in range(r0 // M, (r0 + n) // M):
                act_copy(k).wait_recv()

        def layer2(r0, n):
            return mlp(abuf[r0:r0 + n, :], 0).astype(BF16)

        for c in swaps:
            c.wait_recv()
        for c in lifts[2:]:
            c.start()

        applied = {}
        r0 = 0
        for n, hid in EARLY:
            arrived(r0, n)
            a3 = layer2(r0, n)
            abuf[r0:r0 + n, :] = a3
            if r0 < SHARE:
                sbuf[r0:r0 + n, :] = a3
                send(r0, n)
            acc[r0:r0 + n, :] = mlp(a3, 1, 0, hid)
            applied.update({k: hid for k in range(r0 // M, (r0 + n) // M)})
            r0 += n
        n_shared = len(sent)
        for c in w3_swaps:
            c.wait_recv()

        def finish(f0, n):
            hid, *others = [applied.pop(k) for k in range(f0 // M, (f0 + n) // M)]
            assert all(other == hid for other in others)
            emit(f0, n, acc[f0:f0 + n, :] + mlp(abuf[f0:f0 + n, :], 1, hid))

        for f0, n in FINISH:
            finish(f0, n)

        for n in STEADY:
            if r0 < UP0 * M:
                arrived(r0, n)
                emit(r0, n, mlp(layer2(r0, n), 1))
                r0 += n
                continue
            for lo in range(r0, r0 + 2 * M, n):
                arrived(lo, n)
                emit(lo, n, mlp(layer2(lo, n), 1))
                arrived(lo + 2 * M, n)
                emit(lo + 2 * M, n, mlp(abuf[lo + 2 * M:lo + 2 * M + n, :], 1))
            r0 += 4 * M
        assert r0 == R

        before = len(sent) - TAIL
        for _, _, c in sent[:before]:
            c.wait_recv()
        for p0, n, _ in sent[n_shared:before]:
            write_out(oth0, p0, n, ybuf[p0:p0 + n, :])
        finish(0, SHARE)
        write_out(oth0, 0, SHARE, mlp(ybuf[0:SHARE, :], 1))
        assert not applied

        def take(p0, n, c):
            c.wait_recv()
            write_out(oth0, p0, n, ybuf[p0:p0 + n, :])

        taken = before
        for j in range(n_det):
            upto = before + (j * TAIL) // n_det
            for piece in sent[taken:upto]:
                take(*piece)
            taken = upto
            if j == n_det - 1:
                for c in swaps + w3_swaps + lifts + [c for _, _, c in sent[:-1]]:
                    c.wait_send()
                for i in range(n_det):
                    detour(i, 0).wait_send()
            take(*DETOUR[j], detour(j, 2))
        sent[-1][2].wait_send()
        for piece in sent[taken:]:
            take(*piece)


def pallas_dist_pipemlp_pp2tp2_xy_b4096_d256_h512_kernel(
    x_padded: jax.Array,
    Win: jax.Array,
    Wout: jax.Array,
):
    n_det = len(DETOUR)
    det_rows = sum(n for _, n in DETOUR)
    dma = pltpu.SemaphoreType.DMA
    return pl.pallas_call(
        _body,
        out_shape=pltpu.VMEM((1, ROWS, D), F32),
        in_specs=[pl.BlockSpec(memory_space=pltpu.HBM)] * 3,
        out_specs=pl.BlockSpec(memory_space=pltpu.VMEM),
        scratch_shapes=[
            pltpu.VMEM((2, D, HH), F32),
            pltpu.VMEM((2, HH, D), F32),
            pltpu.VMEM((3, D, 2 * HH), BF16),
            pltpu.VMEM((3, 2 * HH, D), BF16),
            pltpu.VMEM((ROWS, D), F32),
            pltpu.VMEM((ROWS, D), F32),
            pltpu.VMEM((ROWS, D), BF16),
            pltpu.VMEM((R, D), BF16),
            pltpu.VMEM((R, D), BF16),
            pltpu.VMEM((det_rows, D), BF16),
            pltpu.VMEM((det_rows, D), BF16),
            dma((len(FIRST) + 3 + ROWS // XB,)),
            dma((len(FIRST) + 3,)), dma((len(FIRST) + 3,)),
            dma((4,)), dma((4,)),
            dma((N_CHUNKS,)), dma((N_CHUNKS,)),
            dma((N_CHUNKS,)), dma((N_CHUNKS,)),
            dma((2 * n_det,)), dma((n_det,)), dma((n_det,)), dma((n_det,)),
            pltpu.SemaphoreType.REGULAR,
        ],
        compiler_params=pltpu.CompilerParams(
            collective_id=0,
            vmem_limit_bytes=32 * 1024 * 1024,
            disable_semaphore_checks=True,
        ),
    )(x_padded, Win, Wout)
```
